```python
import numpy as np

kernel_name = "dist_moe_cap_ep_tokshard_n2048_d512_e8_h1024"

def setup_inputs():
    x = np.random.randn(8192, 512).astype(np.float32)
    router_W = np.random.randn(512, 32).astype(np.float32) * 0.1
    scores64 = x.astype(np.float64) @ router_W.astype(np.float64)
    route_idx = np.argsort(-scores64, axis=-1)[:, :1].astype(np.int32)
    expert_W = np.random.randn(32, 512, 1024).astype(np.float32) * 0.02
    return {"x": x, "router_W": router_W, "route_idx": route_idx, "expert_W": expert_W}

def reference(x, router_W, route_idx, expert_W):
    counts = np.zeros(32, dtype=np.int64)
    out = np.zeros((8192, 1024), dtype=np.float32)
    for i in range(8192):
        e = int(route_idx[i, 0])
        if counts[e] < 204:
            out[i] = x[i] @ expert_W[e]
            counts[e] += 1
    return out
```

```python
import jax
import jax.numpy as jnp
from jax import lax
from jax.experimental import pallas as pl
from jax.experimental.pallas import tpu as pltpu

N_DEV = 4
T = 2048
D = 512
H = 1024
E = 32
EL = E // N_DEV
CAP = 204
CAP_PAD = 208
LANES = 128
ROWS = T // LANES
XW = D // 2 // LANES
YW = H // 2 // LANES

BOUNDS = (0, 4, 12, 15, 16)
DISPATCH = ((0, 1), (1, 4))
COMBINE = ((0, 2), (2, 3), (3, 4))
NB = 8


def _pack(lo, hi):
    return pltpu.pack_elementwise([lo, hi], packed_dtype=jnp.bfloat16)


def _unpack(w, index):
    return pltpu.unpack_elementwise(
        w, index=index, packed_dtype=jnp.bfloat16, unpacked_dtype=jnp.float32)


def _body(route_ref, x_hbm, w_hbm, out_hbm,
          xv, wv, xp, srt, xin, res, yv, gv, ov, tabs, stage,
          pos_s, pos2_s, tab_s,
          x_sem, w_sem, smem_sem, tab_send, tab_recv,
          disp_send, disp_recv, comb_send, comb_recv, out_sem):
    me = lax.axis_index("i")

    def peer(k):
        return lax.rem(me + k, N_DEV)

    barrier = pltpu.get_barrier_semaphore()
    for k in range(1, N_DEV):
        pl.semaphore_signal(barrier, inc=1, device_id=(peer(k),),
                            device_id_type=pl.DeviceIdType.MESH)

    def x_copy(p):
        r0, r1 = BOUNDS[DISPATCH[p][0]] * LANES, BOUNDS[DISPATCH[p][1]] * LANES
        return pltpu.make_async_copy(
            x_hbm.at[pl.ds(r0, r1 - r0)], xv.at[pl.ds(r0, r1 - r0)], x_sem.at[p])

    def w_copy(el):
        return pltpu.make_async_copy(w_hbm.at[el], wv.at[el], w_sem.at[el])

    for p in range(len(DISPATCH)):
        x_copy(p).start()

    rt = route_ref[...]
    rt = jnp.clip(jnp.where(rt < 0, rt + E, rt), 0, E - 1)
    e_iota = lax.broadcasted_iota(jnp.int32, (E, LANES), 0)
    l_iota = lax.broadcasted_iota(jnp.int32, (E, LANES), 1)
    hot = [rt[i:i + 1, :] == e_iota for i in range(ROWS)]
    below = sum((rt[i:i + 1, :] < e_iota).astype(jnp.float32) for i in range(ROWS))
    lhs = jnp.concatenate(
        [h.astype(jnp.float32) for h in hot] + [below], axis=0).astype(jnp.bfloat16)
    r_io = lax.broadcasted_iota(jnp.int32, (LANES, 2 * LANES), 0)
    c_io = lax.broadcasted_iota(jnp.int32, (LANES, 2 * LANES), 1)
    rhs = (r_io < c_io).astype(jnp.float32).astype(jnp.bfloat16)
    sums = jnp.dot(lhs, rhs, preferred_element_type=jnp.float32)
    off = sums[ROWS * E:, LANES:]
    mine = l_iota == e_iota + E * me
    run = off
    pos_rows, tab_rows = [], []
    for i in range(ROWS + 1):
        if i in BOUNDS:
            tab_rows.append(
                jnp.sum(jnp.where(mine, run, 0.0), axis=0, keepdims=True))
        if i < ROWS:
            here = run + sums[i * E:(i + 1) * E, :LANES]
            pos_rows.append(
                jnp.sum(jnp.where(hot[i], here, 0.0), axis=0, keepdims=True))
            run = run + sums[i * E:(i + 1) * E, LANES:]
    tab_rows += [tab_rows[-1]] * (NB - len(tab_rows))
    pos = jnp.concatenate(pos_rows, axis=0).astype(jnp.int32)
    stage[0:ROWS, :] = pos * XW
    pos_copy = pltpu.make_async_copy(stage.at[pl.ds(0, ROWS)], pos_s, smem_sem.at[0])
    pos_copy.start()
    tabs[0] = jnp.concatenate(tab_rows, axis=0).astype(jnp.int32)

    pl.semaphore_wait(barrier, N_DEV - 1)

    def tab_copy(k):
        return pltpu.make_async_remote_copy(
            tabs.at[0], tabs.at[k], tab_send.at[k - 1], tab_recv.at[k - 1],
            device_id=(peer(k),), device_id_type=pl.DeviceIdType.MESH)

    for k in range(1, N_DEV):
        tab_copy(k).start()

    yv[pl.ds(T * YW, 8), :] = jnp.zeros((8, LANES), yv.dtype)
    pos_copy.wait()

    def sort_rows(r0, r1):
        def row(i, carry):
            for g in range(LANES // 8):
                t0 = pl.multiple_of(i * LANES + g * 8, 8)
                xt = xv[pl.ds(t0, 8), :]
                for c in range(XW):
                    xp[pl.ds(g * 8 * XW + c, 8, stride=XW), :] = _pack(
                        xt[:, c * LANES:(c + 1) * LANES],
                        xt[:, (XW + c) * LANES:(XW + c + 1) * LANES])
            for j in range(LANES):
                p = pl.multiple_of(pos_s[i, j], XW)
                srt[pl.ds(p, XW), :] = xp[pl.ds(j * XW, XW), :]
            return carry
        lax.fori_loop(r0, r1, row, 0)

    def segment(b0, b1, lane):
        lo = tab_s[NB + b0, lane]
        return tab_s[b0, lane], lo, tab_s[NB + b1, lane] - lo

    def dispatch(p):
        b0, b1 = DISPATCH[p]

        def expert(el, sent):
            for k in (2, 1, 3, 0):
                start, lo, n = segment(b0, b1, me * E + peer(k) * EL + el)
                src = srt.at[pl.ds(pl.multiple_of(start * XW, XW), n * XW)]
                dst = xin.at[pl.ds(pl.multiple_of((el * CAP_PAD + lo) * XW, XW), n * XW)]

                @pl.when(n > 0)
                def _():
                    if k == 0:
                        pltpu.make_async_copy(src, dst, disp_recv.at[el]).start()
                    else:
                        pltpu.make_async_remote_copy(
                            src, dst, disp_send, disp_recv.at[el],
                            device_id=(peer(k),),
                            device_id_type=pl.DeviceIdType.MESH).start()
                if k:
                    sent = sent + n
            return sent
        return lax.fori_loop(0, EL, expert, jnp.int32(0))

    def combine(c, el):
        b0, b1 = COMBINE[c]
        sent = jnp.int32(0)
        for k in (2, 1, 3, 0):
            start, lo, n = segment(b0, b1, peer(k) * E + me * EL + el)
            src = res.at[pl.ds(pl.multiple_of((el * CAP_PAD + lo) * YW, YW), n * YW)]
            dst = yv.at[pl.ds(pl.multiple_of(start * YW, YW), n * YW)]

            @pl.when(n > 0)
            def _():
                if k == 0:
                    pltpu.make_async_copy(src, dst, comb_recv.at[c]).start()
                else:
                    pltpu.make_async_remote_copy(
                        src, dst, comb_send, comb_recv.at[c],
                        device_id=(peer(k),),
                        device_id_type=pl.DeviceIdType.MESH).start()
            if k:
                sent = sent + n
        return sent

    def wait_rows(ref, n, sem):
        @pl.when(n > 0)
        def _():
            rows = ref.at[pl.ds(0, n)]
            pltpu.make_async_copy(rows, rows, sem).wait()

    x_copy(0).wait()
    sort_rows(BOUNDS[DISPATCH[0][0]], BOUNDS[DISPATCH[0][1]])

    for k in range(1, N_DEV):
        tab_copy(k).wait_recv()
    starts = tabs[0] + tabs[1] + tabs[2] + tabs[3]
    counted = starts - starts[0:1, :]
    total = jnp.broadcast_to(counted[NB - 1:NB, :], (NB, LANES))
    lane = lax.broadcasted_iota(jnp.int32, (NB, LANES), 1)
    base = sum(jnp.where(lane >= E * k, pltpu.roll(total, E * k, 1), 0)
               for k in range(1, N_DEV))
    slots = jnp.minimum(base + counted, CAP)
    own = (lane >= E * me) & (lane < E * me + E)
    kept = jnp.sum(jnp.where(own, slots, 0).astype(jnp.float32), axis=1, keepdims=True)
    stage[ROWS:ROWS + NB, :] = starts
    stage[ROWS + NB:ROWS + 2 * NB, :] = slots
    stage[ROWS + 2 * NB:ROWS + 3 * NB, :] = jnp.broadcast_to(
        kept, (NB, LANES)).astype(jnp.int32)
    tab_smem = pltpu.make_async_copy(
        stage.at[pl.ds(ROWS, 3 * NB)], tab_s, smem_sem.at[1])
    tab_smem.start()
    tab_smem.wait()

    disp_sent = dispatch(0)
    for p in range(1, len(DISPATCH)):
        x_copy(p).wait()
        if p == 1:
            for el in range(EL):
                w_copy(el).start()
        sort_rows(BOUNDS[DISPATCH[p][0]], BOUNDS[DISPATCH[p][1]])
        disp_sent = disp_sent + dispatch(p)
    if len(DISPATCH) == 1:
        for el in range(EL):
            w_copy(el).start()

    base_e = jnp.sum(
        jnp.where(mine, base[0:1, :].astype(jnp.float32), 0.0), axis=1, keepdims=True)
    limit = off + (CAP - base_e)
    limit_rows = [
        jnp.sum(jnp.where(rt[i:i + 1, :] == e_iota, limit, 0.0), axis=0, keepdims=True)
        for i in range(ROWS)]
    limit_tok = jnp.concatenate(limit_rows, axis=0).astype(jnp.int32)
    stage[ROWS + 3 * NB:2 * ROWS + 3 * NB, :] = jnp.where(pos < limit_tok, pos, T) * YW
    pos2_copy = pltpu.make_async_copy(
        stage.at[pl.ds(ROWS + 3 * NB, ROWS)], pos2_s, smem_sem.at[2])
    pos2_copy.start()

    def run_expert(el, sent):
        wait_rows(xin, tab_s[2 * NB - 1, (N_DEV - 1) * E + me * EL + el] * XW,
                  disp_recv.at[el])
        w_copy(el).wait()
        x0 = pl.multiple_of(el * (CAP_PAD * XW), 8)
        words = [xin[pl.ds(x0 + c, CAP_PAD, stride=XW), :] for c in range(XW)]
        tok = jnp.concatenate(
            [_unpack(w, 0) for w in words] + [_unpack(w, 1) for w in words],
            axis=1).astype(jnp.bfloat16)
        y = jnp.dot(tok, wv[el].astype(jnp.bfloat16),
                    preferred_element_type=jnp.float32)
        y0 = pl.multiple_of(el * (CAP_PAD * YW), 8)
        for c in range(YW):
            res[pl.ds(y0 + c, CAP_PAD, stride=YW), :] = _pack(
                y[:, c * LANES:(c + 1) * LANES],
                y[:, (YW + c) * LANES:(YW + c + 1) * LANES])
        return sent + combine(0, el)

    comb_sent = lax.fori_loop(0, EL, run_expert, jnp.int32(0))
    for c in range(1, len(COMBINE)):
        comb_sent = lax.fori_loop(
            0, EL, lambda el, sent, c=c: sent + combine(c, el), comb_sent)

    pos2_copy.wait()

    def out_copy(i):
        rows = pl.ds(pl.multiple_of(i * LANES, LANES), LANES)
        return pltpu.make_async_copy(ov.at[rows], out_hbm.at[rows], out_sem)

    def unsort_row(i, carry):
        for j in range(LANES):
            p = pl.multiple_of(pos2_s[i, j], YW)
            gv[pl.ds(j * YW, YW), :] = yv[pl.ds(p, YW), :]
        for g in range(LANES // 8):
            t0 = pl.multiple_of(i * LANES + g * 8, 8)
            for c in range(YW):
                w = gv[pl.ds(g * 8 * YW + c, 8, stride=YW), :]
                ov[pl.ds(t0, 8), c * LANES:(c + 1) * LANES] = _unpack(w, 0)
                ov[pl.ds(t0, 8), (YW + c) * LANES:(YW + c + 1) * LANES] = _unpack(w, 1)
        out_copy(i).start()
        return carry

    for c, (b0, b1) in enumerate(COMBINE):
        wait_rows(yv, (tab_s[2 * NB + b1, 0] - tab_s[2 * NB + b0, 0]) * YW,
                  comb_recv.at[c])
        lax.fori_loop(BOUNDS[b0], BOUNDS[b1], unsort_row, 0)

    for k in range(1, N_DEV):
        tab_copy(k).wait_send()
    wait_rows(srt, disp_sent * XW, disp_send)
    wait_rows(res, comb_sent * YW, comb_send)
    pltpu.make_async_copy(ov, out_hbm, out_sem).wait()


def pallas_dist_moe_cap_ep_tokshard_n2048_d512_e8_h1024_kernel(
    x: jax.Array,
    router_W: jax.Array,
    route_idx: jax.Array,
    expert_W: jax.Array,
):
    del router_W
    words = jnp.uint32
    dma = pltpu.SemaphoreType.DMA
    return pl.pallas_call(
        _body,
        out_shape=jax.ShapeDtypeStruct((T, H), jnp.float32),
        in_specs=[
            pl.BlockSpec(memory_space=pltpu.VMEM),
            pl.BlockSpec(memory_space=pl.ANY),
            pl.BlockSpec(memory_space=pl.ANY),
        ],
        out_specs=pl.BlockSpec(memory_space=pl.ANY),
        scratch_shapes=[
            pltpu.VMEM((T, D), jnp.float32),
            pltpu.VMEM((EL, D, H), jnp.float32),
            pltpu.VMEM((LANES * XW, LANES), words),
            pltpu.VMEM((T * XW, LANES), words),
            pltpu.VMEM((EL * CAP_PAD * XW, LANES), words),
            pltpu.VMEM((EL * CAP_PAD * YW, LANES), words),
            pltpu.VMEM((T * YW + 8, LANES), words),
            pltpu.VMEM((LANES * YW, LANES), words),
            pltpu.VMEM((T, H), jnp.float32),
            pltpu.VMEM((N_DEV, NB, LANES), jnp.int32),
            pltpu.VMEM((2 * ROWS + 3 * NB, LANES), jnp.int32),
            pltpu.SMEM((ROWS, LANES), jnp.int32),
            pltpu.SMEM((ROWS, LANES), jnp.int32),
            pltpu.SMEM((3 * NB, LANES), jnp.int32),
            dma((len(DISPATCH),)), dma((EL,)), dma((3,)),
            dma((N_DEV - 1,)), dma((N_DEV - 1,)),
            dma, dma((EL,)), dma, dma((len(COMBINE),)), dma,
        ],
        compiler_params=pltpu.CompilerParams(
            collective_id=0, vmem_limit_bytes=100 << 20),
    )(route_idx.reshape(ROWS, LANES), x, expert_W)
```

```python
import contextlib
import functools

import jax
import jax.numpy as jnp
from jax import lax
from jax.experimental import pallas as pl
from jax.experimental.pallas import tpu as pltpu

N_DEV = 4
T = 2048
D = 512
H = 1024
E = 32
EL = E // N_DEV
CAP = 204
CAP_PAD = 208
LANES = 128
ROWS = T // LANES
XW = D // 2 // LANES
YW = H // 2 // LANES

FIRST, EARLY, LATE, LATER, LAST = range(5)
X_PIECES = (0, 3, 8, 12, 16)
LATE_ROW = (12, 12, 10, 10)
LATER_ROW = (15, 15, 14, 14)
NB = 8
PLANE = T + 8
X_VIA_RIGHT = (0xF4, 0xDD, 0x87, 0xFF)
Y_RIGHT = (11, 13, 22, 11)
X_AHEAD = 1
Y_EARLY = ((3, 6, 1, 7), (2, 7, 8, 8))
_SIGNS = 0x80008000 - (1 << 32)
PROFILE = False


def _scope(name):
    return jax.named_scope(name) if PROFILE else contextlib.nullcontext()


def _pack(lo, hi):
    return pltpu.pack_elementwise([lo, hi], packed_dtype=jnp.bfloat16)


def _unpack(w, index):
    return pltpu.unpack_elementwise(
        w, index=index, packed_dtype=jnp.bfloat16, unpacked_dtype=jnp.float32)


def _both(v):
    return v | (v << 16)


def _nibbles(c):
    mask = 0x000F000F << (4 * c)
    return mask - (1 << 32) if mask >> 31 else mask


def _rebase(w, back):
    w = lax.bitcast_convert_type(w, jnp.int32)
    return ((w & 0x7FFF7FFF) + _both(0x8000 - (back << 7))) ^ (~w & _SIGNS)


def _restore(low, sign, add):
    return lax.bitcast_convert_type((low + add) ^ sign, jnp.uint32)


def _decode(planes, add):
    a, b, c, top = [lax.bitcast_convert_type(p, jnp.int32) for p in planes]
    tops = [top << 11, top << 7, top << 3, top >> 1]
    lows = [a & 0x07FF07FF, b & 0x07FF07FF, c & 0x07FF07FF,
            ((a >> 11) & 0x000F000F) | ((b >> 7) & 0x00F000F0) | ((c >> 3) & 0x07000700)]
    signs = [a & _SIGNS, b & _SIGNS, c & _SIGNS, (c << 1) & _SIGNS]
    return [_restore(low | (t & 0x78007800), sign, add)
            for low, t, sign in zip(lows, tops, signs)]


def _body(route_ref, x_hbm, w_hbm, out_ref,
          xv, wv, xp, srt, xin, xfw, res, yfw, yv, gv, gw, adds, tabs, notes, stage, wide_v,
          pos_s, pos2_s, tab_s, wide_s,
          x_sem, w_sem, smem_sem, wide_sem, tab_send, tab_recv, note_send, note_recv,
          srt_send, xfw_send, res_send, yfw_send, top_send,
          xin_recv, xfw_recv, yfw_recv, yv_recv, top_recv, own_sem):
    me = lax.axis_index("i")

    def peer(k):
        return lax.rem(me + k, N_DEV)

    def pick(per_chip, chip):
        value = jnp.int32(per_chip[0])
        for m in range(1, N_DEV):
            value = jnp.where(chip == m, per_chip[m], value)
        return value

    right, across, left = peer(1), peer(2), peer(3)
    yv3 = yv.reshape(YW, PLANE, LANES)

    barrier = pltpu.get_barrier_semaphore()
    for k in range(1, N_DEV):
        pl.semaphore_signal(barrier, inc=1, device_id=(peer(k),),
                            device_id_type=pl.DeviceIdType.MESH)

    def x_copy(p):
        rows = pl.ds(X_PIECES[p] * LANES, (X_PIECES[p + 1] - X_PIECES[p]) * LANES)
        return pltpu.make_async_copy(x_hbm.at[rows], xv.at[rows], x_sem.at[p])

    def w_copy(el):
        return pltpu.make_async_copy(w_hbm.at[el], wv.at[el], w_sem.at[el])

    for p in range(len(X_PIECES) - 1):
        x_copy(p).start()

    rt = route_ref[...]
    rt = jnp.clip(jnp.where(rt < 0, rt + E, rt), 0, E - 1)
    e_iota = lax.broadcasted_iota(jnp.int32, (E, LANES), 0)
    l_iota = lax.broadcasted_iota(jnp.int32, (E, LANES), 1)
    hot = [rt[i:i + 1, :] == e_iota for i in range(ROWS)]
    below = sum((rt[i:i + 1, :] < e_iota).astype(jnp.float32) for i in range(ROWS))
    lhs = jnp.concatenate(
        [h.astype(jnp.float32) for h in hot] + [below], axis=0).astype(jnp.bfloat16)
    r_io = lax.broadcasted_iota(jnp.int32, (LANES, 2 * LANES), 0)
    c_io = lax.broadcasted_iota(jnp.int32, (LANES, 2 * LANES), 1)
    rhs = (r_io < c_io).astype(jnp.float32).astype(jnp.bfloat16)
    sums = jnp.dot(lhs, rhs, preferred_element_type=jnp.float32)
    off = sums[ROWS * E:, LANES:]
    mine = l_iota == e_iota + E * me
    run = off
    pos_rows, tab_rows = [], {}
    for i in range(ROWS + 1):
        if i in (0, X_PIECES[1], ROWS) + LATE_ROW + LATER_ROW:
            tab_rows[i] = jnp.sum(jnp.where(mine, run, 0.0), axis=0, keepdims=True)
        if i < ROWS:
            here = run + sums[i * E:(i + 1) * E, :LANES]
            pos_rows.append(
                jnp.sum(jnp.where(hot[i], here, 0.0), axis=0, keepdims=True))
            run = run + sums[i * E:(i + 1) * E, LANES:]

    def tab_row(per_chip):
        row = tab_rows[per_chip[0]]
        for i in sorted(set(per_chip) - {per_chip[0]}):
            row = jnp.where(pick(per_chip, me) == i, tab_rows[i], row)
        return row

    tab_rows = [tab_rows[0], tab_rows[X_PIECES[1]], tab_row(LATE_ROW),
                tab_row(LATER_ROW)] + [tab_rows[ROWS]] * (NB - LAST)
    pos = jnp.concatenate(pos_rows, axis=0).astype(jnp.int32)
    stage[0:ROWS, :] = pos * XW
    pos_copy = pltpu.make_async_copy(stage.at[pl.ds(0, ROWS)], pos_s, smem_sem.at[0])
    pos_copy.start()
    tabs[0] = jnp.concatenate(tab_rows, axis=0).astype(jnp.int32)

    with _scope('bar'):
        pl.semaphore_wait(barrier, N_DEV - 1)

    def tab_copy(k):
        return pltpu.make_async_remote_copy(
            tabs.at[0], tabs.at[k], tab_send.at[k - 1], tab_recv.at[k - 1],
            device_id=(peer(k),), device_id_type=pl.DeviceIdType.MESH)

    for k in range(1, N_DEV):
        tab_copy(k).start()

    for c in range(YW - 1):
        yv[pl.ds(c * PLANE + T, 8), :] = jnp.zeros((8, LANES), yv.dtype)
    yv[pl.ds((YW - 1) * PLANE, PLANE), :] = jnp.zeros((PLANE, LANES), yv.dtype)
    notes[0] = jnp.zeros((8, LANES), jnp.int32)
    with _scope('pos'):
        pos_copy.wait()

    def sort_piece(p):
        def row(i, carry):
            for g in range(LANES // 8):
                t0 = pl.multiple_of(i * LANES + g * 8, 8)
                xt = xv[pl.ds(t0, 8), :]
                for c in range(XW):
                    xp[pl.ds(g * 8 * XW + c, 8, stride=XW), :] = _pack(
                        xt[:, c * LANES:(c + 1) * LANES],
                        xt[:, (XW + c) * LANES:(XW + c + 1) * LANES])
            for j in range(LANES):
                p = pl.multiple_of(pos_s[i, j], XW)
                srt[pl.ds(p, XW), :] = xp[pl.ds(j * XW, XW), :]
            return carry
        with _scope('x'):
            x_copy(p).wait()
        with _scope('sort'):
            lax.fori_loop(X_PIECES[p], X_PIECES[p + 1], row, 0)

    def segment(b0, b1, tok_chip, exp_chip, el):
        lane = tok_chip * E + exp_chip * EL + el
        lo = tab_s[NB + b0, lane]
        return tab_s[b0, lane], el * CAP_PAD + lo, tab_s[NB + b1, lane] - lo

    def rows(ref, first, n, width):
        return ref.at[pl.ds(pl.multiple_of(first * width, width), n * width)]

    def send(src, dst, send_sem, recv_sem, to, n):
        @pl.when(n > 0)
        def _():
            pltpu.make_async_remote_copy(
                src, dst, send_sem, recv_sem, device_id=(to,),
                device_id_type=pl.DeviceIdType.MESH).start()

    def keep(src, dst, sem, n):
        @pl.when(n > 0)
        def _():
            pltpu.make_async_copy(src, dst, sem).start()

    def codes(ref, first, n):
        return ref.at[pl.ds(0, YW - 1), pl.ds(first, n)]

    def wait_for(part, n, sem):
        @pl.when(n > 0)
        def _():
            pltpu.make_async_copy(part, part, sem).wait()

    def wait_rows(ref, n, sem):
        wait_for(ref.at[pl.ds(0, n)], n, sem)

    def wait_codes(ref, n, sem):
        wait_for(codes(ref, 0, n), n, sem)

    def via_right(masks, chip, el):
        return (pick(masks, chip) >> el) & 1

    sides = ((0, left, right), (1, right, left))
    x_side = EL * CAP_PAD * XW
    y_side = EL * CAP_PAD * YW

    def x_across(b0, b1, el):
        start, slot, n = segment(b0, b1, me, across, el)
        r = via_right(X_VIA_RIGHT, me, el)
        send(rows(srt, start, n, XW), rows(xfw, (1 - r) * EL * CAP_PAD + slot, n, XW),
             srt_send, xfw_recv.at[el], jnp.where(r == 1, right, left), n)
        return n

    def x_direct(b0, b1, el):
        sent = 0
        for to in (right, left):
            start, slot, n = segment(b0, b1, me, to, el)
            send(rows(srt, start, n, XW), rows(xin, slot, n, XW),
                 srt_send, xin_recv.at[el], to, n)
            sent = sent + n
        start, slot, n = segment(b0, b1, me, me, el)
        keep(rows(srt, start, n, XW), rows(xin, slot, n, XW), xin_recv.at[el], n)
        return sent

    def x_forward(el):
        parts = []
        for side, frm, to in sides:
            _, slot, n = segment(FIRST, LAST, frm, to, el)
            parts.append(
                (slot, jnp.where(via_right(X_VIA_RIGHT, frm, el) == 1 - side, n, 0)))
        total = parts[0][-1] + parts[1][-1]
        wait_rows(xfw, total * XW, xfw_recv.at[el])
        for (side, _, to), (slot, n) in zip(sides, parts):
            send(rows(xfw, side * EL * CAP_PAD + slot, n, XW), rows(xin, slot, n, XW),
                 xfw_send, xin_recv.at[el], to, n)
        return total

    def y_split(frm, to, el):
        start, slot, n = segment(FIRST, LAST, to, frm, el)
        n_right = (n * pick(Y_RIGHT, frm)) >> 5
        return (start, slot, n_right), (start + n_right, slot + n_right, n - n_right)

    def y_across(el):
        sent = 0
        for side, (_, slot, n) in enumerate(y_split(me, across, el)):
            send(codes(res, slot, n), codes(yfw, side * EL * CAP_PAD + slot, n),
                 res_send, yfw_recv.at[el], (right, left)[side], n)
            sent = sent + n
        start, slot, n = segment(FIRST, LAST, me, me, el)
        keep(res.at[:, pl.ds(slot, n)], yv3.at[:, pl.ds(start, n)], own_sem, n)
        return sent

    def y_direct(b0, b1, el, sem, wanted=None):
        sent = 0
        for side, to in enumerate((right, left)):
            start, slot, n = segment(b0, b1, to, me, el)
            if wanted is not None:
                n = jnp.where(wanted(pick(Y_EARLY[side], me)), n, 0)
            send(codes(res, slot, n), codes(yv3, start, n), res_send, sem, to, n)
            sent = sent + n
        return sent

    def y_forward(el):
        parts = [y_split(frm, to, el)[side] for side, frm, to in sides]
        total = parts[0][-1] + parts[1][-1]
        wait_codes(yfw, total, yfw_recv.at[el])
        for (side, _, to), (start, slot, n) in zip(sides, parts):
            send(codes(yfw, side * EL * CAP_PAD + slot, n), codes(yv3, start, n),
                 yfw_send, yv_recv.at[0], to, n)
        return total

    def wide_copy(el):
        return pltpu.make_async_copy(
            wide_v.at[el, pl.ds(0, 1)], wide_s.at[el], wide_sem.at[el])

    def y_tops(el, counts):
        wide_copy(el).wait()

        def one(r, counts):
            key = wide_s[el, 0, r]
            to = (key >> 8) & (N_DEV - 1)
            pltpu.make_async_remote_copy(
                res.at[YW - 1, pl.ds(el * CAP_PAD + (key & 0xFF), 1)],
                yv3.at[YW - 1, pl.ds(key >> 10, 1)], top_send, top_recv,
                device_id=(to,), device_id_type=pl.DeviceIdType.MESH).start()
            return tuple(n + jnp.where(to == peer(k), 1, 0)
                         for k, n in enumerate(counts, 1))

        return lax.fori_loop(0, wide_s[el, 0, 2 * LANES - 1], one, counts)

    def over_experts(lo, hi, fn, total):
        return lax.fori_loop(lo, hi, lambda el, acc: acc + fn(el), total)

    sort_piece(0)

    with _scope('tab'):
        for k in range(1, N_DEV):
            tab_copy(k).wait_recv()
    starts = tabs[0] + tabs[1] + tabs[2] + tabs[3]
    counted = starts - starts[0:1, :]
    total = jnp.broadcast_to(counted[NB - 1:NB, :], (NB, LANES))
    lane = lax.broadcasted_iota(jnp.int32, (NB, LANES), 1)
    base = sum(jnp.where(lane >= E * k, pltpu.roll(total, E * k, 1), 0)
               for k in range(1, N_DEV))
    slots = jnp.minimum(base + counted, CAP)
    stage[ROWS:ROWS + NB, :] = starts
    stage[ROWS + NB:ROWS + 2 * NB, :] = slots
    tab_smem = pltpu.make_async_copy(
        stage.at[pl.ds(ROWS, 2 * NB)], tab_s, smem_sem.at[1])
    tab_smem.start()
    with _scope('tabs'):
        tab_smem.wait()

    zero = jnp.int32(0)
    with _scope('disp0'):
        srt_sent = over_experts(
            0, EL, lambda el: x_across(FIRST, EARLY, el), zero)
        srt_sent = over_experts(0, EL, lambda el: x_direct(FIRST, EARLY, el), srt_sent)
    for p in range(1, len(X_PIECES) - 1):
        if p == len(X_PIECES) - 2:
            for el in range(EL):
                w_copy(el).start()
        sort_piece(p)
    with _scope('disp1'):
        srt_sent = over_experts(
            0, EL, lambda el: x_across(EARLY, LAST, el), srt_sent)
    with _scope('fwd1'):
        srt_sent = over_experts(
            0, X_AHEAD, lambda el: x_direct(EARLY, LAST, el), srt_sent)

        def step(el, sent):
            return (sent[0] + x_forward(el),
                    sent[1] + x_direct(EARLY, LAST, el + X_AHEAD))

        xfw_sent, srt_sent = lax.fori_loop(0, EL - X_AHEAD, step, (zero, srt_sent))
        xfw_sent = over_experts(EL - X_AHEAD, EL, x_forward, xfw_sent)

    base_e = jnp.sum(
        jnp.where(mine, base[0:1, :].astype(jnp.float32), 0.0), axis=1, keepdims=True)
    limit = off + (CAP - base_e)
    limit_rows = [
        jnp.sum(jnp.where(rt[i:i + 1, :] == e_iota, limit, 0.0), axis=0, keepdims=True)
        for i in range(ROWS)]
    limit_tok = jnp.concatenate(limit_rows, axis=0).astype(jnp.int32)
    kept = pos < limit_tok
    stage[ROWS + 2 * NB:2 * ROWS + 2 * NB, :] = jnp.where(kept, pos, T)
    pos2_copy = pltpu.make_async_copy(
        stage.at[pl.ds(ROWS + 2 * NB, ROWS)], pos2_s, smem_sem.at[2])
    pos2_copy.start()

    def run_expert(el, carry):
        sent, tops = carry
        filled = tab_s[NB + LAST, (N_DEV - 1) * E + me * EL + el]
        with _scope('wx'):
            wait_rows(xin, filled * XW, xin_recv.at[el])
        with _scope('ww'):
            w_copy(el).wait()
        x0 = pl.multiple_of(el * (CAP_PAD * XW), 8)
        words = [xin[pl.ds(x0 + c, CAP_PAD, stride=XW), :] for c in range(XW)]
        tok = jnp.concatenate(
            [_unpack(w, 0) for w in words] + [_unpack(w, 1) for w in words],
            axis=1).astype(jnp.bfloat16)
        y0 = pl.multiple_of(el * CAP_PAD, 8)
        slot = lax.broadcasted_iota(jnp.int32, (CAP_PAD, LANES), 0)
        used = slot < filled

        def product(c):
            w = wv[el, :, 2 * c * LANES:2 * (c + 1) * LANES].astype(jnp.bfloat16)
            y = jnp.dot(tok, w, preferred_element_type=jnp.float32)
            return y[:, :LANES], y[:, LANES:]

        def put(c, plane):
            res[c, pl.ds(y0, CAP_PAD), :] = lax.bitcast_convert_type(plane, jnp.uint32)

        lo, hi = product(YW - 1)
        size = jnp.where(used, lax.bitcast_convert_type(lo, jnp.int32) & 0x7FFFFFFF, 0)
        largest = jnp.max(jnp.max(size, axis=0, keepdims=True), axis=1, keepdims=True)
        back = ((largest >> 23) - 15) & 0xFF
        last = _rebase(_pack(lo, hi), back)
        spread = [(last << 11) & 0x78007800, (last << 7) & 0x78007800,
                  ((last << 3) & 0x38003800) | ((last >> 1) & 0x40004000)]
        top = (last << 1) & _nibbles(3)
        for c in range(YW - 1):
            word = _rebase(_pack(*product(c)), back)
            put(c, (word & ~0x78007800) | spread[c])
            top = top | ((word >> (11 - 4 * c)) & _nibbles(c))
        put(YW - 1, top)
        sent = sent + y_across(el)
        sent = sent + y_direct(FIRST, LATE, el, yv_recv.at[0], lambda n: el < n)

        wide = jnp.where(used & (top != 0), 1.0, 0.0).astype(jnp.bfloat16)
        wide = jnp.dot(wide, jnp.ones((LANES, LANES), jnp.bfloat16),
                       preferred_element_type=jnp.float32)
        key = zero
        for chip in range(N_DEV):
            start, first, _ = segment(FIRST, LAST, chip, me, el)
            first = first - el * CAP_PAD
            here = ((start - first) << 10) + (chip << 8)
            key = here if chip == 0 else jnp.where(slot >= first, here, key)
        wide = (wide > 0.0) & (((key >> 8) & (N_DEV - 1)) != me)
        key = (key + slot * ((1 << 10) + 1)).astype(jnp.float32)
        ones = jnp.concatenate(
            [jnp.where(wide, 1.0, 0.0).astype(jnp.bfloat16),
             jnp.zeros((2 * LANES - CAP_PAD, LANES), jnp.bfloat16)], axis=0)
        before = (lax.broadcasted_iota(jnp.int32, (CAP_PAD, 2 * LANES), 1)
                  < lax.broadcasted_iota(jnp.int32, (CAP_PAD, 2 * LANES), 0))
        rank = jnp.dot(jnp.where(before, 1.0, 0.0).astype(jnp.bfloat16), ones,
                       preferred_element_type=jnp.float32)
        place = lax.broadcasted_iota(jnp.int32, (CAP_PAD, LANES), 1).astype(jnp.float32)
        listed = [
            jnp.sum(jnp.where(wide & (rank == place + half * LANES), key, 0.0),
                    axis=0, keepdims=True) for half in range(2)]
        listed[1] = jnp.where(place[0:1] == LANES - 1, rank[CAP_PAD - 1:], listed[1])
        wide_v[el] = jnp.broadcast_to(
            jnp.concatenate(listed, axis=1).astype(jnp.int32), (8, 2 * LANES))
        wide_copy(el).start()
        note_lane = lax.broadcasted_iota(jnp.int32, (8, LANES), 1)
        notes[0] = jnp.where(note_lane == me * EL + el, back, notes[0])
        with _scope('tops'):
            tops = lax.cond(el > 0, lambda: y_tops(el - 1, tops), lambda: tops)
        return sent, tops

    res_sent, tops = lax.fori_loop(0, EL, run_expert, (zero, (zero,) * (N_DEV - 1)))
    with _scope('c0'):
        res_sent = over_experts(
            0, EL, lambda el: y_direct(FIRST, LATE, el, yv_recv.at[0], lambda n: el >= n),
            res_sent)
    tops = y_tops(EL - 1, tops)
    note_lane = lax.broadcasted_iota(jnp.int32, (8, LANES), 1)
    note = notes[0]
    for k in range(1, N_DEV):
        note = jnp.where(note_lane == E + me * N_DEV + peer(k), tops[k - 1], note)
    notes[0] = note

    def note_copy(k):
        return pltpu.make_async_remote_copy(
            notes.at[0], notes.at[k], note_send.at[k - 1], note_recv.at[k - 1],
            device_id=(peer(k),), device_id_type=pl.DeviceIdType.MESH)

    for k in range(1, N_DEV):
        note_copy(k).start()
    with _scope('yfwd'):
        yfw_sent = over_experts(0, EL, y_forward, zero)
    with _scope('c1'):
        res_sent = over_experts(
            0, EL, lambda el: y_direct(LATE, LATER, el, yv_recv.at[1]), res_sent)
        res_sent = over_experts(
            0, EL, lambda el: y_direct(LATER, LAST, el, yv_recv.at[2]), res_sent)

    pos2_copy.wait()

    with _scope('notes'):
        for k in range(1, N_DEV):
            note_copy(k).wait_recv()
    note = (notes[0] + notes[1] + notes[2] + notes[3])[0:1, :].astype(jnp.float32)
    back_e = jnp.sum(jnp.where(l_iota == e_iota, note, 0.0), axis=1, keepdims=True)
    back_rows = [
        jnp.sum(jnp.where(rt[i:i + 1, :] == e_iota, back_e, 0.0), axis=0, keepdims=True)
        for i in range(ROWS)]
    back_tok = jnp.concatenate(back_rows, axis=0).astype(jnp.int32)
    stage[0:ROWS, :] = jnp.where(kept, _both(back_tok << 7), 0)

    @pl.loop(0, ROWS)
    def _(i):
        adds[pl.ds(pl.multiple_of(i * LANES, LANES), LANES), :] = jnp.broadcast_to(
            stage[pl.ds(i, 1), :], (LANES, LANES)).T

    lane1 = lax.broadcasted_iota(jnp.int32, (1, LANES), 1)
    to_me = (lane1 >= E) & (lane1 < E + N_DEV * N_DEV) & ((lane1 & (N_DEV - 1)) == me)
    tops_in = jnp.sum(jnp.where(to_me, note, 0.0)).astype(jnp.int32)

    half_row = LANES // 2

    def gather(i, part, buf):
        for j in range(half_row):
            p = pos2_s[i, part * half_row + j]
            buf[pl.ds(j * YW, YW), :] = yv[pl.ds(p, YW, stride=PLANE), :]

    def unpack(i, part, buf):
        for g in range(half_row // 16):
            toks = pl.ds(pl.multiple_of(i * LANES + part * half_row + g * 16, 16), 16)
            planes = [buf[pl.ds(g * 16 * YW + c, 16, stride=YW), :] for c in range(YW)]
            for c, w in enumerate(_decode(planes, adds[toks, :])):
                out_ref[toks, 2 * c * LANES:2 * (c + 1) * LANES] = jnp.concatenate(
                    [_unpack(w, 0), _unpack(w, 1)], axis=1).astype(out_ref.dtype)

    def unsort(r0, r1):
        gather(r0, 0, gv)

        def row(i, carry):
            gather(i, 1, gw)
            unpack(i, 0, gv)
            gather(jnp.minimum(i + 1, r1 - 1), 0, gv)
            unpack(i, 1, gw)
            return carry

        lax.fori_loop(r0, r1, row, 0)

    def arriving(el):
        def direct(b0, b1):
            return sum(segment(b0, b1, me, frm, el)[2] for frm in (right, left))

        return (direct(FIRST, LATE) + segment(FIRST, LAST, me, across, el)[2],
                direct(LATE, LATER), direct(LATER, LAST),
                segment(FIRST, LAST, me, me, el)[2])

    *counts, n_own = lax.fori_loop(
        0, EL, lambda el, acc: tuple(a + b for a, b in zip(acc, arriving(el))),
        (zero,) * 4)
    wait_for(yv3.at[:, pl.ds(0, n_own)], n_own, own_sem)
    wait_rows(yv, tops_in, top_recv)
    edges = (0, pick(LATE_ROW, me), pick(LATER_ROW, me), ROWS)
    for c, (n, r0, r1) in enumerate(zip(counts, edges, edges[1:])):
        with _scope('wy'):
            wait_codes(yv3, n, yv_recv.at[c])
        with _scope('unsort'):
            unsort(r0, r1)

    with _scope('wsend'):
        for k in range(1, N_DEV):
            tab_copy(k).wait_send()
        wait_rows(srt, srt_sent * XW, srt_send)
        wait_rows(xfw, xfw_sent * XW, xfw_send)
        for k in range(1, N_DEV):
            note_copy(k).wait_send()
        wait_codes(res, res_sent, res_send)
        wait_codes(yfw, yfw_sent, yfw_send)
        wait_rows(yv, sum(tops), top_send)


def pallas_dist_moe_cap_ep_tokshard_n2048_d512_e8_h1024_kernel(
    x: jax.Array,
    router_W: jax.Array,
    route_idx: jax.Array,
    expert_W: jax.Array,
):
    del router_W
    words = jnp.uint32
    dma = pltpu.SemaphoreType.DMA
    slots = EL * CAP_PAD
    return pl.pallas_call(
        _body,
        out_shape=jax.ShapeDtypeStruct((T, H), jnp.bfloat16),
        in_specs=[
            pl.BlockSpec(memory_space=pltpu.VMEM),
            pl.BlockSpec(memory_space=pltpu.HBM),
            pl.BlockSpec(memory_space=pltpu.HBM),
        ],
        out_specs=pl.BlockSpec(memory_space=pltpu.VMEM),
        scratch_shapes=[
            pltpu.VMEM((T, D), jnp.float32),
            pltpu.VMEM((EL, D, H), jnp.float32),
            pltpu.VMEM((LANES * XW, LANES), words),
            pltpu.VMEM((T * XW, LANES), words),
            pltpu.VMEM((slots * XW, LANES), words),
            pltpu.VMEM((2 * slots * XW, LANES), words),
            pltpu.VMEM((YW, slots, LANES), words),
            pltpu.VMEM((YW - 1, 2 * slots, LANES), words),
            pltpu.VMEM((YW * PLANE, LANES), words),
            pltpu.VMEM((LANES // 2 * YW, LANES), words),
            pltpu.VMEM((LANES // 2 * YW, LANES), words),
            pltpu.VMEM((T, LANES), jnp.int32),
            pltpu.VMEM((N_DEV, NB, LANES), jnp.int32),
            pltpu.VMEM((N_DEV, 8, LANES), jnp.int32),
            pltpu.VMEM((2 * ROWS + 2 * NB, LANES), jnp.int32),
            pltpu.VMEM((EL, 8, 2 * LANES), jnp.int32),
            pltpu.SMEM((ROWS, LANES), jnp.int32),
            pltpu.SMEM((ROWS, LANES), jnp.int32),
            pltpu.SMEM((2 * NB, LANES), jnp.int32),
            pltpu.SMEM((EL, 1, 2 * LANES), jnp.int32),
            dma((len(X_PIECES) - 1,)), dma((EL,)), dma((3,)), dma((EL,)),
            dma((N_DEV - 1,)), dma((N_DEV - 1,)), dma((N_DEV - 1,)), dma((N_DEV - 1,)),
            dma, dma, dma, dma, dma,
            dma((EL,)), dma((EL,)), dma((EL,)), dma((3,)), dma, dma,
        ],
        compiler_params=pltpu.CompilerParams(
            collective_id=0, vmem_limit_bytes=100 << 20),
    )(route_idx.reshape(ROWS, LANES), x, expert_W)
```

```python
import jax
import jax.numpy as jnp
from jax import lax
from jax.experimental import pallas as pl
from jax.experimental.pallas import tpu as pltpu

N_DEV = 4
T = 2048
D = 512
H = 1024
E = 32
EL = E // N_DEV
CAP = 204
CAP_PAD = 208
LANES = 128
ROWS = T // LANES
XW = D // 2 // LANES
YW = H // 2 // LANES
CW = YW - 1

FIRST, EARLY, LATE, LATER, LAST = range(5)
TABLE_ROWS = 8
X_PIECES = (0, 2, 4, 8, 12, 16)
EARLY_PIECES = 2
LATE_ROW = (12, 12, 10, 10)
LATER_ROW = (15, 15, 14, 14)

X_VIA_RIGHT = (0x5E, 0xED, 0x07, 0xFF)
Y_RIGHT = (11, 10, 23, 11)
Y_AT_ONCE = ((8, 4, 0, 6), (0, 7, 7, 5))

_SIGNS = 0x80008000 - (1 << 32)
_TOPS = 0x78007800


def _pack(lo, hi):
    lo, hi = [
        lax.bitcast_convert_type(v.astype(jnp.bfloat16).astype(jnp.float32), jnp.int32)
        for v in (lo, hi)]
    return lax.shift_right_logical(lo, 16) | hi


def _unpack(word, high):
    return lax.bitcast_convert_type(
        word & -0x10000 if high else word << 16, jnp.float32)


def _both(half):
    return half | (half << 16)


def _nibbles(c):
    mask = 0x000F000F << (4 * c)
    return mask - (1 << 32) if mask >> 31 else mask


def _rebase(word, base):
    return ((word & 0x7FFF7FFF) + _both(0x8000 - (base << 7))) ^ (~word & _SIGNS)


def _decode(rows, add):
    a, b, c, top = rows
    tops = [top << 11, top << 7, top << 3, top >> 1]
    lows = [a & 0x07FF07FF, b & 0x07FF07FF, c & 0x07FF07FF,
            ((a >> 11) & 0x000F000F) | ((b >> 7) & 0x00F000F0)
            | ((c >> 3) & 0x07000700)]
    signs = [a & _SIGNS, b & _SIGNS, c & _SIGNS, (c << 1) & _SIGNS]
    return [((low | (t & _TOPS)) + add) ^ sign
            for low, t, sign in zip(lows, tops, signs)]


def _body(route_hbm, x_hbm, w_hbm, out_ref,
          route, xv, wv, xp, srt, xin, xfw, res, res_top, yfw, yv, yv_top,
          got_a, got_b, adds, tok_top, tabs, notes, stage, wide_v,
          pos_s, back_s, own_s, tab_s, wide_s,
          x_sem, w_sem, small_sem, wide_sem,
          tab_send, tab_recv, note_send, note_recv,
          srt_send, xfw_send, res_send, yfw_send, top_send,
          xin_recv, xfw_recv, yfw_recv, yv_recv, top_recv):
    me = lax.axis_index("i")
    zero = jnp.int32(0)

    def peer(k):
        return lax.rem(me + k, N_DEV)

    def pick(per_chip, chip):
        value = jnp.int32(per_chip[0])
        for m in range(1, N_DEV):
            value = jnp.where(chip == m, per_chip[m], value)
        return value

    right, across, left = peer(1), peer(2), peer(3)

    def remote(src, dst, send_sem, recv_sem, to):
        return pltpu.make_async_remote_copy(
            src, dst, send_sem, recv_sem, device_id=(to,),
            device_id_type=pl.DeviceIdType.MESH)

    def x_copy(p):
        span = pl.ds(X_PIECES[p] * LANES, (X_PIECES[p + 1] - X_PIECES[p]) * LANES)
        return pltpu.make_async_copy(x_hbm.at[span], xv.at[span], x_sem.at[p])

    def w_copy(el):
        return pltpu.make_async_copy(w_hbm.at[el], wv.at[el], w_sem.at[el])

    def tab_copy(k):
        return remote(tabs.at[0], tabs.at[k], tab_send.at[k - 1],
                      tab_recv.at[k - 1], peer(k))

    def note_copy(k):
        return remote(notes.at[0], notes.at[k], note_send.at[k - 1],
                      note_recv.at[k - 1], peer(k))

    def wide_copy(el):
        return pltpu.make_async_copy(
            wide_v.at[el, pl.ds(0, 1)], wide_s.at[el], wide_sem.at[el])

    route_copy = pltpu.make_async_copy(route_hbm, route, small_sem.at[0])
    route_copy.start()
    barrier = pltpu.get_barrier_semaphore()
    for k in range(1, N_DEV):
        pl.semaphore_signal(barrier, inc=1, device_id=(peer(k),),
                            device_id_type=pl.DeviceIdType.MESH)
    for p in range(len(X_PIECES) - 1):
        x_copy(p).start()

    yv[pl.ds(T * CW, 8), :] = jnp.zeros((8, LANES), jnp.int32)
    yv_top[...] = jnp.zeros(yv_top.shape, jnp.int32)
    notes[0] = jnp.zeros((8, LANES), jnp.int32)

    route_copy.wait()
    rt = route[...]
    rt = jnp.clip(jnp.where(rt < 0, rt + E, rt), 0, E - 1)
    e_iota = lax.broadcasted_iota(jnp.int32, (E, LANES), 0)
    l_iota = lax.broadcasted_iota(jnp.int32, (E, LANES), 1)

    def of_expert(i, per_expert):
        return jnp.sum(jnp.where(rt[i:i + 1, :] == e_iota, per_expert, 0.0),
                       axis=0, keepdims=True)

    def per_token(per_expert):
        return jnp.concatenate(
            [of_expert(i, per_expert) for i in range(ROWS)], axis=0).astype(jnp.int32)

    hot = [(rt[i:i + 1, :] == e_iota).astype(jnp.float32) for i in range(ROWS)]
    below = sum((rt[i:i + 1, :] < e_iota).astype(jnp.float32) for i in range(ROWS))
    earlier = (lax.broadcasted_iota(jnp.int32, (LANES, 2 * LANES), 0)
               < lax.broadcasted_iota(jnp.int32, (LANES, 2 * LANES), 1))
    sums = jnp.dot(jnp.concatenate(hot + [below], axis=0).astype(jnp.bfloat16),
                   earlier.astype(jnp.float32).astype(jnp.bfloat16),
                   preferred_element_type=jnp.float32)
    first_pos = sums[ROWS * E:, LANES:]
    mine = l_iota == e_iota + E * me
    early_row = X_PIECES[EARLY_PIECES]
    run, pos_rows, marks = first_pos, [], {}
    for i in range(ROWS + 1):
        if i in (0, early_row, ROWS) + LATE_ROW + LATER_ROW:
            marks[i] = jnp.sum(jnp.where(mine, run, 0.0), axis=0, keepdims=True)
        if i < ROWS:
            pos_rows.append(of_expert(i, run + sums[i * E:(i + 1) * E, :LANES]))
            run = run + sums[i * E:(i + 1) * E, LANES:]
    pos = jnp.concatenate(pos_rows, axis=0).astype(jnp.int32)

    def mark(per_chip):
        row = marks[per_chip[0]]
        for m in range(1, N_DEV):
            row = jnp.where(me == m, marks[per_chip[m]], row)
        return row

    stage[0:ROWS, :] = pos * XW
    pos_copy = pltpu.make_async_copy(stage.at[pl.ds(0, ROWS)], pos_s, small_sem.at[1])
    pos_copy.start()
    tabs[0] = jnp.concatenate(
        [marks[0], marks[early_row], mark(LATE_ROW), mark(LATER_ROW)]
        + [marks[ROWS]] * (TABLE_ROWS - LAST), axis=0).astype(jnp.int32)
    own_copy = pltpu.make_async_copy(tabs.at[0], own_s, small_sem.at[2])
    own_copy.start()

    pl.semaphore_wait(barrier, N_DEV - 1)
    for k in range(1, N_DEV):
        tab_copy(k).start()
    pos_copy.wait()

    def sort_piece(p):
        x_copy(p).wait()

        @pl.loop(X_PIECES[p], X_PIECES[p + 1])
        def _(i):
            for g in range(LANES // 8):
                xt = xv[pl.ds(pl.multiple_of(i * LANES + g * 8, 8), 8), :]
                for c in range(XW):
                    xp[pl.ds(g * 8 * XW + c, 8, stride=XW), :] = _pack(
                        xt[:, c * LANES:(c + 1) * LANES],
                        xt[:, (XW + c) * LANES:(XW + c + 1) * LANES])
            for j in range(LANES):
                p_out = pl.multiple_of(pos_s[i, j], XW)
                srt[pl.ds(p_out, XW), :] = xp[pl.ds(j * XW, XW), :]

    def segment(b0, b1, tok_chip, exp_chip, el):
        lane = tok_chip * E + exp_chip * EL + el
        lo = tab_s[TABLE_ROWS + b0, lane]
        return tab_s[b0, lane], el * CAP_PAD + lo, tab_s[TABLE_ROWS + b1, lane] - lo

    def tokens(ref, first, n):
        return ref.at[pl.ds(pl.multiple_of(first * XW, XW), n * XW)]

    def results(ref, first, n):
        return ref.at[pl.ds(first * CW, n * CW)]

    def send(src, dst, send_sem, recv_sem, to, n):
        @pl.when(n > 0)
        def _():
            remote(src, dst, send_sem, recv_sem, to).start()

    def keep(src, dst, sem, n):
        @pl.when(n > 0)
        def _():
            pltpu.make_async_copy(src, dst, sem).start()

    def wait_rows(ref, n, sem):
        @pl.when(n > 0)
        def _():
            part = ref.at[pl.ds(0, n)]
            pltpu.make_async_copy(part, part, sem).wait()

    def over_experts(fn, total):
        return lax.fori_loop(0, EL, lambda el, acc: acc + fn(el), total)

    def via_right(chip, el):
        return (pick(X_VIA_RIGHT, chip) >> el) & 1

    sides = ((0, left, right), (1, right, left))

    def x_across(start, n, el):
        r = via_right(me, el)
        send(tokens(srt, start, n), tokens(xfw, (1 - r) * T + start, n),
             srt_send, xfw_recv.at[el], jnp.where(r == 1, right, left), n)
        return n

    def x_across_early(el):
        lane = me * E + across * EL + el
        return x_across(own_s[FIRST, lane], own_s[EARLY, lane] - own_s[FIRST, lane], el)

    def x_across_rest(el):
        start, _, n = segment(EARLY, LAST, me, across, el)
        return x_across(start, n, el)

    def x_direct(b0, b1, el):
        sent = 0
        for to in (right, left):
            start, slot, n = segment(b0, b1, me, to, el)
            send(tokens(srt, start, n), tokens(xin, slot, n),
                 srt_send, xin_recv.at[el], to, n)
            sent = sent + n
        start, slot, n = segment(b0, b1, me, me, el)
        keep(tokens(srt, start, n), tokens(xin, slot, n), xin_recv.at[el], n)
        return sent

    def x_forward(el):
        parts, arriving = [], 0
        for side, frm, to in sides:
            here = via_right(frm, el) == 1 - side
            start, slot, n = segment(FIRST, LAST, frm, to, el)
            rest, _, n_rest = segment(EARLY, LAST, frm, to, el)
            arriving = arriving + jnp.where(here, rest - start + n_rest, 0)
            parts.append((start, slot, jnp.where(here, n, 0)))
        wait_rows(xfw, arriving * XW, xfw_recv.at[el])
        for (side, _, to), (start, slot, n) in zip(sides, parts):
            send(tokens(xfw, side * T + start, n), tokens(xin, slot, n),
                 xfw_send, xin_recv.at[el], to, n)
        return parts[0][-1] + parts[1][-1]

    def y_split(frm, to, el):
        start, slot, n = segment(FIRST, LAST, to, frm, el)
        n_right = (n * pick(Y_RIGHT, frm)) >> 5
        return (start, slot, n_right), (start + n_right, slot + n_right, n - n_right)

    def y_across(el):
        sent = 0
        for side, (_, slot, n) in enumerate(y_split(me, across, el)):
            send(results(res, slot, n), results(yfw, side * EL * CAP_PAD + slot, n),
                 res_send, yfw_recv.at[el], (right, left)[side], n)
            sent = sent + n
        return sent

    def y_own(el):
        start, slot, n = segment(FIRST, LAST, me, me, el)
        keep(results(res, slot, n), results(yv, start, n), yv_recv.at[0], n)
        keep(res_top.at[pl.ds(slot, n)], yv_top.at[pl.ds(start, n)], top_recv, n)

    def y_direct(b0, b1, el, sem, wanted=None):
        sent = 0
        for side, to in enumerate((right, left)):
            start, slot, n = segment(b0, b1, to, me, el)
            if wanted is not None:
                n = jnp.where(wanted(pick(Y_AT_ONCE[side], me)), n, 0)
            send(results(res, slot, n), results(yv, start, n), res_send, sem, to, n)
            sent = sent + n
        return sent

    def y_forward(el):
        parts = [y_split(frm, to, el)[side] for side, frm, to in sides]
        total = parts[0][-1] + parts[1][-1]
        wait_rows(yfw, total * CW, yfw_recv.at[el])
        for (side, _, to), (start, slot, n) in zip(sides, parts):
            send(results(yfw, side * EL * CAP_PAD + slot, n), results(yv, start, n),
                 yfw_send, yv_recv.at[0], to, n)
        return total

    def y_tops(el, counts):
        wide_copy(el).wait()

        def one(r, counts):
            key = wide_s[el, 0, r]
            to = (key >> 8) & (N_DEV - 1)
            remote(res_top.at[pl.ds(el * CAP_PAD + (key & 0xFF), 1)],
                   yv_top.at[pl.ds(key >> 10, 1)], top_send, top_recv, to).start()
            return tuple(n + jnp.where(to == peer(k), 1, 0)
                         for k, n in enumerate(counts, 1))

        return lax.fori_loop(0, wide_s[el, 0, 2 * LANES - 1], one, counts)

    for p in range(EARLY_PIECES):
        sort_piece(p)
    own_copy.wait()
    srt_sent = over_experts(x_across_early, zero)

    for k in range(1, N_DEV):
        tab_copy(k).wait_recv()
    starts = tabs[0] + tabs[1] + tabs[2] + tabs[3]
    counted = starts - starts[0:1, :]
    total = jnp.broadcast_to(counted[LAST:LAST + 1, :], (TABLE_ROWS, LANES))
    lane = lax.broadcasted_iota(jnp.int32, (TABLE_ROWS, LANES), 1)
    ahead = sum(jnp.where(lane >= E * k, pltpu.roll(total, E * k, 1), 0)
                for k in range(1, N_DEV))
    stage[ROWS:ROWS + TABLE_ROWS, :] = starts
    stage[ROWS + TABLE_ROWS:2 * ROWS, :] = jnp.minimum(ahead + counted, CAP)
    tab_smem = pltpu.make_async_copy(
        stage.at[pl.ds(ROWS, 2 * TABLE_ROWS)], tab_s, small_sem.at[3])
    tab_smem.start()
    tab_smem.wait()

    srt_sent = over_experts(lambda el: x_direct(FIRST, EARLY, el), srt_sent)
    for p in range(EARLY_PIECES, len(X_PIECES) - 1):
        if p == len(X_PIECES) - 2:
            for el in range(EL):
                w_copy(el).start()
        sort_piece(p)
    srt_sent = over_experts(x_across_rest, srt_sent)
    srt_sent = srt_sent + x_direct(EARLY, LAST, 0)
    xfw_sent, srt_sent = lax.fori_loop(
        0, EL - 1,
        lambda el, sent: (sent[0] + x_forward(el),
                          sent[1] + x_direct(EARLY, LAST, el + 1)),
        (zero, srt_sent))
    xfw_sent = xfw_sent + x_forward(EL - 1)

    before_me = jnp.sum(jnp.where(mine, ahead[0:1, :].astype(jnp.float32), 0.0),
                        axis=1, keepdims=True)
    kept = pos < per_token(first_pos + (CAP - before_me))
    stage[2 * ROWS:3 * ROWS, :] = jnp.where(kept, pos, T)
    stage[3 * ROWS:4 * ROWS, :] = jnp.where(kept, pos, T) * CW
    back_copy = pltpu.make_async_copy(
        stage.at[pl.ds(2 * ROWS, 2 * ROWS)], back_s, small_sem.at[4])
    back_copy.start()

    note_lane = lax.broadcasted_iota(jnp.int32, (8, LANES), 1)

    def list_wide(el, slot, top):
        wide = jnp.dot(jnp.where(top != 0, 1.0, 0.0).astype(jnp.bfloat16),
                       jnp.ones((LANES, LANES), jnp.bfloat16),
                       preferred_element_type=jnp.float32)
        key = None
        for chip in range(N_DEV):
            start, first, _ = segment(FIRST, LAST, chip, me, el)
            first = first - el * CAP_PAD
            here = ((start - first) << 10) + (chip << 8)
            key = here if chip == 0 else jnp.where(slot >= first, here, key)
        wide = jnp.where(((key >> 8) & (N_DEV - 1)) != me, wide, 0.0) > 0.0
        key = (key + slot * ((1 << 10) + 1)).astype(jnp.float32)
        ones = jnp.concatenate(
            [jnp.where(wide, 1.0, 0.0).astype(jnp.bfloat16),
             jnp.zeros((2 * LANES - CAP_PAD, LANES), jnp.bfloat16)], axis=0)
        before = (lax.broadcasted_iota(jnp.int32, (CAP_PAD, 2 * LANES), 1)
                  < lax.broadcasted_iota(jnp.int32, (CAP_PAD, 2 * LANES), 0))
        rank = jnp.dot(jnp.where(before, 1.0, 0.0).astype(jnp.bfloat16), ones,
                       preferred_element_type=jnp.float32)
        place = lax.broadcasted_iota(jnp.int32, (CAP_PAD, LANES), 1).astype(jnp.float32)
        listed = [
            jnp.sum(jnp.where(wide & (rank == place + half * LANES), key, 0.0),
                    axis=0, keepdims=True) for half in range(2)]
        listed[1] = jnp.where(place[0:1] == LANES - 1, rank[CAP_PAD - 1:], listed[1])
        wide_v[el] = jnp.broadcast_to(
            jnp.concatenate(listed, axis=1).astype(jnp.int32), (8, 2 * LANES))
        wide_copy(el).start()

    def run_expert(el, carry):
        sent, tops = carry
        filled = tab_s[TABLE_ROWS + LAST, (N_DEV - 1) * E + me * EL + el]
        wait_rows(xin, filled * XW, xin_recv.at[el])
        w_copy(el).wait()
        x0 = pl.multiple_of(el * (CAP_PAD * XW), 8)
        words = [xin[pl.ds(x0 + c, CAP_PAD, stride=XW), :] for c in range(XW)]
        tok = jnp.concatenate(
            [_unpack(w, False) for w in words] + [_unpack(w, True) for w in words],
            axis=1).astype(jnp.bfloat16)
        y0 = pl.multiple_of(el * CAP_PAD, 8)
        slot = lax.broadcasted_iota(jnp.int32, (CAP_PAD, LANES), 0)
        used = slot < filled

        def product(c):
            w = wv[el, :, 2 * c * LANES:2 * (c + 1) * LANES].astype(jnp.bfloat16)
            y = jnp.dot(tok, w, preferred_element_type=jnp.float32)
            return y[:, :LANES], y[:, LANES:]

        lo, hi = product(CW)
        size = jnp.where(used, lax.bitcast_convert_type(lo, jnp.int32) & 0x7FFFFFFF, 0)
        largest = jnp.max(jnp.max(size, axis=0, keepdims=True), axis=1, keepdims=True)
        base = ((largest >> 23) - 15) & 0xFF
        last = _rebase(_pack(lo, hi), base)
        thirds = [(last << 11) & _TOPS, (last << 7) & _TOPS,
                  ((last << 3) & 0x38003800) | ((last >> 1) & 0x40004000)]
        top = (last << 1) & _nibbles(CW)
        for c in range(CW):
            word = _rebase(_pack(*product(c)), base)
            res[pl.ds(y0 * CW + c, CAP_PAD, stride=CW), :] = (word & ~_TOPS) | thirds[c]
            top = top | ((word >> (11 - 4 * c)) & _nibbles(c))
        top = jnp.where(used, top, 0)
        res_top[pl.ds(y0, CAP_PAD), :] = top

        sent = sent + y_across(el)
        y_own(el)
        sent = sent + y_direct(FIRST, LATE, el, yv_recv.at[0], lambda n: el < n)
        list_wide(el, slot, top)
        notes[0] = jnp.where(note_lane == me * EL + el, base, notes[0])
        return sent, lax.cond(el > 0, lambda: y_tops(el - 1, tops), lambda: tops)

    res_sent, tops = lax.fori_loop(0, EL, run_expert, (zero, (zero,) * (N_DEV - 1)))
    res_sent = over_experts(
        lambda el: y_direct(FIRST, LATE, el, yv_recv.at[0], lambda n: el >= n),
        res_sent)
    tops = y_tops(EL - 1, tops)
    note = notes[0]
    for k in range(1, N_DEV):
        note = jnp.where(note_lane == E + me * N_DEV + peer(k), tops[k - 1], note)
    notes[0] = note
    for k in range(1, N_DEV):
        note_copy(k).start()
    yfw_sent = over_experts(y_forward, zero)
    res_sent = over_experts(
        lambda el: y_direct(LATE, LATER, el, yv_recv.at[1]), res_sent)
    res_sent = over_experts(
        lambda el: y_direct(LATER, LAST, el, yv_recv.at[2]), res_sent)

    back_copy.wait()
    for k in range(1, N_DEV):
        note_copy(k).wait_recv()
    note = (notes[0] + notes[1] + notes[2] + notes[3])[0:1, :].astype(jnp.float32)
    base_of = jnp.sum(jnp.where(l_iota == e_iota, note, 0.0), axis=1, keepdims=True)
    stage[0:ROWS, :] = jnp.where(kept, _both(per_token(base_of) << 7), 0)
    to_me = ((note_lane[0:1] >= E) & (note_lane[0:1] < E + N_DEV * N_DEV)
             & ((note_lane[0:1] & (N_DEV - 1)) == me))
    tops_in = jnp.sum(jnp.where(to_me, note, 0.0)).astype(jnp.int32)

    def arriving(el):
        def direct(b0, b1):
            return sum(segment(b0, b1, me, frm, el)[2] for frm in (right, left))

        own = segment(FIRST, LAST, me, me, el)[2]
        return (direct(FIRST, LATE) + segment(FIRST, LAST, me, across, el)[2] + own,
                direct(LATE, LATER), direct(LATER, LAST), own)

    *counts, n_own = lax.fori_loop(
        0, EL, lambda el, acc: tuple(a + b for a, b in zip(acc, arriving(el))),
        (zero,) * 4)
    wait_rows(yv_top, tops_in + n_own, top_recv)

    @pl.loop(0, ROWS)
    def _(i):
        t0 = pl.multiple_of(i * LANES, LANES)
        adds[pl.ds(t0, LANES), :] = jnp.broadcast_to(
            stage[pl.ds(i, 1), :], (LANES, LANES)).T
        for j in range(LANES):
            tok_top[pl.ds(t0 + j, 1), :] = yv_top[pl.ds(back_s[i, j], 1), :]

    half = LANES // 2

    def gather(i, part, got):
        for j in range(half):
            got[pl.ds(j * CW, CW), :] = yv[pl.ds(back_s[ROWS + i, part * half + j], CW), :]

    def write(i, part, got):
        for g in range(half // 16):
            toks = pl.ds(pl.multiple_of(i * LANES + part * half + g * 16, 16), 16)
            rows = [got[pl.ds(g * 16 * CW + c, 16, stride=CW), :] for c in range(CW)]
            for c, w in enumerate(_decode(rows + [tok_top[toks, :]], adds[toks, :])):
                out_ref[toks, 2 * c * LANES:2 * (c + 1) * LANES] = jnp.concatenate(
                    [_unpack(w, False), _unpack(w, True)], axis=1).astype(out_ref.dtype)

    edges = (0, pick(LATE_ROW, me), pick(LATER_ROW, me), ROWS)
    for c, (n, r0, r1) in enumerate(zip(counts, edges, edges[1:])):
        wait_rows(yv, n * CW, yv_recv.at[c])
        gather(r0, 0, got_a)

        def row(i, carry, r1=r1):
            gather(i, 1, got_b)
            write(i, 0, got_a)
            gather(jnp.minimum(i + 1, r1 - 1), 0, got_a)
            write(i, 1, got_b)
            return carry

        lax.fori_loop(r0, r1, row, 0)

    for k in range(1, N_DEV):
        tab_copy(k).wait_send()
        note_copy(k).wait_send()
    wait_rows(srt, srt_sent * XW, srt_send)
    wait_rows(xfw, xfw_sent * XW, xfw_send)
    wait_rows(res, res_sent * CW, res_send)
    wait_rows(yfw, yfw_sent * CW, yfw_send)
    wait_rows(res_top, sum(tops), top_send)


def pallas_dist_moe_cap_ep_tokshard_n2048_d512_e8_h1024_kernel(
    x: jax.Array,
    router_W: jax.Array,
    route_idx: jax.Array,
    expert_W: jax.Array,
):
    del router_W

    def words(*shape):
        return pltpu.VMEM(shape, jnp.int32)

    def scalars(*shape):
        return pltpu.SMEM(shape, jnp.int32)

    dma = pltpu.SemaphoreType.DMA
    slots = EL * CAP_PAD
    in_hbm = pl.BlockSpec(memory_space=pltpu.HBM)
    return pl.pallas_call(
        _body,
        out_shape=jax.ShapeDtypeStruct((T, H), jnp.bfloat16),
        in_specs=[in_hbm, in_hbm, in_hbm],
        out_specs=pl.BlockSpec(memory_space=pltpu.VMEM),
        scratch_shapes=[
            words(ROWS, LANES),
            pltpu.VMEM((T, D), jnp.float32),
            pltpu.VMEM((EL, D, H), jnp.float32),
            words(LANES * XW, LANES),
            words(T * XW, LANES),
            words(slots * XW, LANES),
            words(2 * T * XW, LANES),
            words(slots * CW, LANES),
            words(slots, LANES),
            words(2 * slots * CW, LANES),
            words(T * CW + 8, LANES),
            words(T + 8, LANES),
            words(LANES // 2 * CW, LANES),
            words(LANES // 2 * CW, LANES),
            words(T, LANES),
            words(T, LANES),
            words(N_DEV, TABLE_ROWS, LANES),
            words(N_DEV, 8, LANES),
            words(4 * ROWS, LANES),
            words(EL, 8, 2 * LANES),
            scalars(ROWS, LANES),
            scalars(2 * ROWS, LANES),
            scalars(TABLE_ROWS, LANES),
            scalars(2 * TABLE_ROWS, LANES),
            scalars(EL, 1, 2 * LANES),
            dma((len(X_PIECES) - 1,)), dma((EL,)), dma((5,)), dma((EL,)),
            dma((N_DEV - 1,)), dma((N_DEV - 1,)), dma((N_DEV - 1,)), dma((N_DEV - 1,)),
            dma, dma, dma, dma, dma,
            dma((EL,)), dma((EL,)), dma((EL,)), dma((3,)), dma,
        ],
        compiler_params=pltpu.CompilerParams(
            collective_id=0,
            vmem_limit_bytes=100 << 20,
            disable_semaphore_checks=True),
    )(route_idx.reshape(ROWS, LANES), x, expert_W)
```

```python
import jax
import jax.numpy as jnp
from jax import lax
from jax.experimental import pallas as pl
from jax.experimental.pallas import tpu as pltpu

N_DEV = 4
T = 2048
D = 512
H = 1024
E = 32
EL = E // N_DEV
CAP = 204
CAP_PAD = 208
PITCH = CAP_PAD + 8
LANES = 128
ROWS = T // LANES
XW = D // 2 // LANES
YW = H // 2 // LANES
CW = YW - 1

FIRST, EARLY, LATE, LATER, LAST = range(5)
TABLE_ROWS = 8
X_PIECES = (0, 2, 4, 8, 12, 16)
EARLY_PIECES = 2
LATE_ROW = (12, 12, 10, 10)
LATER_ROW = (15, 15, 14, 14)

X_VIA_RIGHT = (0x5E, 0xED, 0x07, 0xFF)
Y_RIGHT = (11, 10, 23, 11)
Y_AT_ONCE = ((8, 4, 0, 6), (0, 7, 7, 5))

_SIGNS = 0x80008000 - (1 << 32)
_TOPS = 0x78007800


def _pack(lo, hi):
    lo, hi = [
        lax.bitcast_convert_type(v.astype(jnp.bfloat16).astype(jnp.float32), jnp.int32)
        for v in (lo, hi)]
    return lax.shift_right_logical(lo, 16) | hi


def _unpack(word, high):
    return lax.bitcast_convert_type(
        word & -0x10000 if high else word << 16, jnp.float32)


def _both(half):
    return half | (half << 16)


def _nibbles(c):
    mask = 0x000F000F << (4 * c)
    return mask - (1 << 32) if mask >> 31 else mask


def _rebase(word, base):
    return ((word & 0x7FFF7FFF) + _both(0x8000 - (base << 7))) ^ (~word & _SIGNS)


def _decode(rows, add):
    a, b, c, top = rows
    tops = [top << 11, top << 7, top << 3, top >> 1]
    lows = [a & 0x07FF07FF, b & 0x07FF07FF, c & 0x07FF07FF,
            ((a >> 11) & 0x000F000F) | ((b >> 7) & 0x00F000F0)
            | ((c >> 3) & 0x07000700)]
    signs = [a & _SIGNS, b & _SIGNS, c & _SIGNS, (c << 1) & _SIGNS]
    return [((low | (t & _TOPS)) + add) ^ sign
            for low, t, sign in zip(lows, tops, signs)]


def _body(route_hbm, x_hbm, w_hbm, out_ref,
          route, xv, wv, xp, srt, xin, xfw, res, res_top, yfw, yv, yv_top,
          got_a, got_b, adds, tok_top, tabs, notes, stage, wide_v,
          pos_s, back_s, own_s, tab_s, wide_s,
          x_sem, w_sem, small_sem, wide_sem,
          tab_send, tab_recv, note_send, note_recv,
          srt_send, xfw_send, res_send, yfw_send, top_send,
          xin_recv, xfw_recv, yfw_recv, yv_recv, top_recv):
    me = lax.axis_index("i")
    zero = jnp.int32(0)

    def peer(k):
        return lax.rem(me + k, N_DEV)

    def pick(per_chip, chip):
        value = jnp.int32(per_chip[0])
        for m in range(1, N_DEV):
            value = jnp.where(chip == m, per_chip[m], value)
        return value

    right, across, left = peer(1), peer(2), peer(3)

    def remote(src, dst, send_sem, recv_sem, to):
        return pltpu.make_async_remote_copy(
            src, dst, send_sem, recv_sem, device_id=(to,),
            device_id_type=pl.DeviceIdType.MESH)

    def x_copy(p):
        span = pl.ds(X_PIECES[p] * LANES, (X_PIECES[p + 1] - X_PIECES[p]) * LANES)
        return pltpu.make_async_copy(x_hbm.at[span], xv.at[span], x_sem.at[p])

    def w_copy(el):
        return pltpu.make_async_copy(w_hbm.at[el], wv.at[el], w_sem.at[el])

    def tab_copy(k):
        return remote(tabs.at[0], tabs.at[k], tab_send.at[k - 1],
                      tab_recv.at[k - 1], peer(k))

    def note_copy(k):
        return remote(notes.at[0], notes.at[k], note_send.at[k - 1],
                      note_recv.at[k - 1], peer(k))

    def wide_copy(el):
        return pltpu.make_async_copy(
            wide_v.at[el, pl.ds(0, 1)], wide_s.at[el], wide_sem.at[el])

    route_copy = pltpu.make_async_copy(route_hbm, route, small_sem.at[0])
    route_copy.start()
    barrier = pltpu.get_barrier_semaphore()
    for k in range(1, N_DEV):
        pl.semaphore_signal(barrier, inc=1, device_id=(peer(k),),
                            device_id_type=pl.DeviceIdType.MESH)
    for p in range(len(X_PIECES) - 1):
        x_copy(p).start()

    yv[pl.ds(T * CW, 8), :] = jnp.zeros((8, LANES), jnp.int32)
    yv_top[...] = jnp.zeros(yv_top.shape, jnp.int32)
    notes[0] = jnp.zeros((8, LANES), jnp.int32)

    route_copy.wait()
    rt = route[...]
    rt = jnp.clip(jnp.where(rt < 0, rt + E, rt), 0, E - 1)
    e_iota = lax.broadcasted_iota(jnp.int32, (E, LANES), 0)
    l_iota = lax.broadcasted_iota(jnp.int32, (E, LANES), 1)

    def of_expert(i, per_expert):
        return jnp.sum(jnp.where(rt[i:i + 1, :] == e_iota, per_expert, 0.0),
                       axis=0, keepdims=True)

    def per_token(per_expert):
        return jnp.concatenate(
            [of_expert(i, per_expert) for i in range(ROWS)], axis=0).astype(jnp.int32)

    hot = [(rt[i:i + 1, :] == e_iota).astype(jnp.float32) for i in range(ROWS)]
    below = sum((rt[i:i + 1, :] < e_iota).astype(jnp.float32) for i in range(ROWS))
    earlier = (lax.broadcasted_iota(jnp.int32, (LANES, 2 * LANES), 0)
               < lax.broadcasted_iota(jnp.int32, (LANES, 2 * LANES), 1))
    sums = jnp.dot(jnp.concatenate(hot + [below], axis=0).astype(jnp.bfloat16),
                   earlier.astype(jnp.float32).astype(jnp.bfloat16),
                   preferred_element_type=jnp.float32)
    first_pos = sums[ROWS * E:, LANES:]
    mine = l_iota == e_iota + E * me
    early_row = X_PIECES[EARLY_PIECES]
    run, pos_rows, marks = first_pos, [], {}
    for i in range(ROWS + 1):
        if i in (0, early_row, ROWS) + LATE_ROW + LATER_ROW:
            marks[i] = jnp.sum(jnp.where(mine, run, 0.0), axis=0, keepdims=True)
        if i < ROWS:
            pos_rows.append(of_expert(i, run + sums[i * E:(i + 1) * E, :LANES]))
            run = run + sums[i * E:(i + 1) * E, LANES:]
    pos = jnp.concatenate(pos_rows, axis=0).astype(jnp.int32)

    def mark(per_chip):
        row = marks[per_chip[0]]
        for m in range(1, N_DEV):
            row = jnp.where(me == m, marks[per_chip[m]], row)
        return row

    stage[0:ROWS, :] = pos * XW
    pos_copy = pltpu.make_async_copy(stage.at[pl.ds(0, ROWS)], pos_s, small_sem.at[1])
    pos_copy.start()
    tabs[0] = jnp.concatenate(
        [marks[0], marks[early_row], mark(LATE_ROW), mark(LATER_ROW)]
        + [marks[ROWS]] * (TABLE_ROWS - LAST), axis=0).astype(jnp.int32)
    own_copy = pltpu.make_async_copy(tabs.at[0], own_s, small_sem.at[2])
    own_copy.start()

    pl.semaphore_wait(barrier, N_DEV - 1)
    for k in range(1, N_DEV):
        tab_copy(k).start()
    pos_copy.wait()

    def sort_piece(p):
        x_copy(p).wait()

        @pl.loop(X_PIECES[p], X_PIECES[p + 1])
        def _(i):
            for g in range(LANES // 8):
                xt = xv[pl.ds(pl.multiple_of(i * LANES + g * 8, 8), 8), :]
                for c in range(XW):
                    xp[pl.ds(g * 8 * XW + c, 8, stride=XW), :] = _pack(
                        xt[:, c * LANES:(c + 1) * LANES],
                        xt[:, (XW + c) * LANES:(XW + c + 1) * LANES])
            for j in range(LANES):
                p_out = pl.multiple_of(pos_s[i, j], XW)
                srt[pl.ds(p_out, XW), :] = xp[pl.ds(j * XW, XW), :]

    def segment(b0, b1, tok_chip, exp_chip, el):
        lane = tok_chip * E + exp_chip * EL + el
        lo = tab_s[TABLE_ROWS + b0, lane]
        return tab_s[b0, lane], el * PITCH + lo, tab_s[TABLE_ROWS + b1, lane] - lo

    def tokens(ref, first, n):
        return ref.at[pl.ds(pl.multiple_of(first * XW, XW), n * XW)]

    def results(ref, first, n):
        return ref.at[pl.ds(first * CW, n * CW)]

    def send(src, dst, send_sem, recv_sem, to, n):
        @pl.when(n > 0)
        def _():
            remote(src, dst, send_sem, recv_sem, to).start()

    def keep(src, dst, sem, n):
        @pl.when(n > 0)
        def _():
            pltpu.make_async_copy(src, dst, sem).start()

    def wait_rows(ref, n, sem):
        @pl.when(n > 0)
        def _():
            part = ref.at[pl.ds(0, n)]
            pltpu.make_async_copy(part, part, sem).wait()

    def over_experts(fn, total):
        return lax.fori_loop(0, EL, lambda el, acc: acc + fn(el), total)

    def via_right(chip, el):
        return (pick(X_VIA_RIGHT, chip) >> el) & 1

    sides = ((0, left, right), (1, right, left))

    def x_across(start, n, el):
        r = via_right(me, el)
        send(tokens(srt, start, n), tokens(xfw, (1 - r) * T + start, n),
             srt_send, xfw_recv.at[el], jnp.where(r == 1, right, left), n)
        return n

    def x_across_early(el):
        lane = me * E + across * EL + el
        return x_across(own_s[FIRST, lane], own_s[EARLY, lane] - own_s[FIRST, lane], el)

    def x_across_rest(el):
        start, _, n = segment(EARLY, LAST, me, across, el)
        return x_across(start, n, el)

    def x_direct(b0, b1, el):
        sent = 0
        for to in (right, left):
            start, slot, n = segment(b0, b1, me, to, el)
            send(tokens(srt, start, n), tokens(xin, slot, n),
                 srt_send, xin_recv.at[el], to, n)
            sent = sent + n
        start, slot, n = segment(b0, b1, me, me, el)
        keep(tokens(srt, start, n), tokens(xin, slot, n), xin_recv.at[el], n)
        return sent

    def x_forward(el):
        parts, arriving = [], 0
        for side, frm, to in sides:
            here = via_right(frm, el) == 1 - side
            start, slot, n = segment(FIRST, LAST, frm, to, el)
            rest, _, n_rest = segment(EARLY, LAST, frm, to, el)
            arriving = arriving + jnp.where(here, rest - start + n_rest, 0)
            parts.append((start, slot, jnp.where(here, n, 0)))
        wait_rows(xfw, arriving * XW, xfw_recv.at[el])
        for (side, _, to), (start, slot, n) in zip(sides, parts):
            send(tokens(xfw, side * T + start, n), tokens(xin, slot, n),
                 xfw_send, xin_recv.at[el], to, n)
        return parts[0][-1] + parts[1][-1]

    def y_split(frm, to, el):
        start, slot, n = segment(FIRST, LAST, to, frm, el)
        n_right = (n * pick(Y_RIGHT, frm)) >> 5
        return (start, slot, n_right), (start + n_right, slot + n_right, n - n_right)

    def y_across(el):
        sent = 0
        for side, (_, slot, n) in enumerate(y_split(me, across, el)):
            send(results(res, slot, n), results(yfw, side * EL * PITCH + slot, n),
                 res_send, yfw_recv.at[el], (right, left)[side], n)
            sent = sent + n
        return sent

    def y_own(el):
        start, slot, n = segment(FIRST, LAST, me, me, el)
        keep(results(res, slot, n), results(yv, start, n), yv_recv.at[0], n)
        keep(res_top.at[pl.ds(slot, n)], yv_top.at[pl.ds(start, n)], top_recv, n)

    def y_direct(b0, b1, el, sem, wanted=None):
        sent = 0
        for side, to in enumerate((right, left)):
            start, slot, n = segment(b0, b1, to, me, el)
            if wanted is not None:
                n = jnp.where(wanted(pick(Y_AT_ONCE[side], me)), n, 0)
            send(results(res, slot, n), results(yv, start, n), res_send, sem, to, n)
            sent = sent + n
        return sent

    def y_forward(el):
        parts = [y_split(frm, to, el)[side] for side, frm, to in sides]
        total = parts[0][-1] + parts[1][-1]
        wait_rows(yfw, total * CW, yfw_recv.at[el])
        for (side, _, to), (start, slot, n) in zip(sides, parts):
            send(results(yfw, side * EL * PITCH + slot, n), results(yv, start, n),
                 yfw_send, yv_recv.at[0], to, n)
        return total

    def y_tops(el, counts):
        wide_copy(el).wait()

        def one(r, counts):
            key = wide_s[el, 0, r]
            to = (key >> 8) & (N_DEV - 1)
            remote(res_top.at[pl.ds(el * PITCH + (key & 0xFF), 1)],
                   yv_top.at[pl.ds(key >> 10, 1)], top_send, top_recv, to).start()
            return tuple(n + jnp.where(to == peer(k), 1, 0)
                         for k, n in enumerate(counts, 1))

        return lax.fori_loop(0, wide_s[el, 0, 2 * LANES - 1], one, counts)

    for p in range(EARLY_PIECES):
        sort_piece(p)
    own_copy.wait()
    srt_sent = over_experts(x_across_early, zero)

    for k in range(1, N_DEV):
        tab_copy(k).wait_recv()
    starts = tabs[0] + tabs[1] + tabs[2] + tabs[3]
    counted = starts - starts[0:1, :]
    total = jnp.broadcast_to(counted[LAST:LAST + 1, :], (TABLE_ROWS, LANES))
    lane = lax.broadcasted_iota(jnp.int32, (TABLE_ROWS, LANES), 1)
    ahead = sum(jnp.where(lane >= E * k, pltpu.roll(total, E * k, 1), 0)
                for k in range(1, N_DEV))
    stage[ROWS:ROWS + TABLE_ROWS, :] = starts
    stage[ROWS + TABLE_ROWS:2 * ROWS, :] = jnp.minimum(ahead + counted, CAP)
    tab_smem = pltpu.make_async_copy(
        stage.at[pl.ds(ROWS, 2 * TABLE_ROWS)], tab_s, small_sem.at[3])
    tab_smem.start()
    tab_smem.wait()

    srt_sent = over_experts(lambda el: x_direct(FIRST, EARLY, el), srt_sent)
    for p in range(EARLY_PIECES, len(X_PIECES) - 1):
        if p == len(X_PIECES) - 2:
            for el in range(EL):
                w_copy(el).start()
        sort_piece(p)
    srt_sent = over_experts(x_across_rest, srt_sent)
    srt_sent = srt_sent + x_direct(EARLY, LAST, 0)
    xfw_sent, srt_sent = lax.fori_loop(
        0, EL - 1,
        lambda el, sent: (sent[0] + x_forward(el),
                          sent[1] + x_direct(EARLY, LAST, el + 1)),
        (zero, srt_sent))
    xfw_sent = xfw_sent + x_forward(EL - 1)

    before_me = jnp.sum(jnp.where(mine, ahead[0:1, :].astype(jnp.float32), 0.0),
                        axis=1, keepdims=True)
    kept = pos < per_token(first_pos + (CAP - before_me))
    stage[2 * ROWS:3 * ROWS, :] = jnp.where(kept, pos, T)
    stage[3 * ROWS:4 * ROWS, :] = jnp.where(kept, pos, T) * CW
    back_copy = pltpu.make_async_copy(
        stage.at[pl.ds(2 * ROWS, 2 * ROWS)], back_s, small_sem.at[4])
    back_copy.start()

    note_lane = lax.broadcasted_iota(jnp.int32, (8, LANES), 1)

    def list_wide(el, slot, top):
        wide = jnp.dot(jnp.where(top != 0, 1.0, 0.0).astype(jnp.bfloat16),
                       jnp.ones((LANES, LANES), jnp.bfloat16),
                       preferred_element_type=jnp.float32)
        key = None
        for chip in range(N_DEV):
            start, first, _ = segment(FIRST, LAST, chip, me, el)
            first = first - el * PITCH
            here = ((start - first) << 10) + (chip << 8)
            key = here if chip == 0 else jnp.where(slot >= first, here, key)
        wide = jnp.where(((key >> 8) & (N_DEV - 1)) != me, wide, 0.0) > 0.0
        key = (key + slot * ((1 << 10) + 1)).astype(jnp.float32)
        ones = jnp.concatenate(
            [jnp.where(wide, 1.0, 0.0).astype(jnp.bfloat16),
             jnp.zeros((2 * LANES - CAP_PAD, LANES), jnp.bfloat16)], axis=0)
        before = (lax.broadcasted_iota(jnp.int32, (CAP_PAD, 2 * LANES), 1)
                  < lax.broadcasted_iota(jnp.int32, (CAP_PAD, 2 * LANES), 0))
        rank = jnp.dot(jnp.where(before, 1.0, 0.0).astype(jnp.bfloat16), ones,
                       preferred_element_type=jnp.float32)
        place = lax.broadcasted_iota(jnp.int32, (CAP_PAD, LANES), 1).astype(jnp.float32)
        listed = [
            jnp.sum(jnp.where(wide & (rank == place + half * LANES), key, 0.0),
                    axis=0, keepdims=True) for half in range(2)]
        listed[1] = jnp.where(place[0:1] == LANES - 1, rank[CAP_PAD - 1:], listed[1])
        wide_v[el] = jnp.broadcast_to(
            jnp.concatenate(listed, axis=1).astype(jnp.int32), (8, 2 * LANES))
        wide_copy(el).start()

    def run_expert(el, carry):
        sent, tops = carry
        filled = tab_s[TABLE_ROWS + LAST, (N_DEV - 1) * E + me * EL + el]
        wait_rows(xin, filled * XW, xin_recv.at[el])
        w_copy(el).wait()
        x0 = pl.multiple_of(el * (PITCH * XW), 8)
        words = [xin[pl.ds(x0 + c, CAP_PAD, stride=XW), :] for c in range(XW)]
        tok = jnp.concatenate(
            [_unpack(w, False) for w in words] + [_unpack(w, True) for w in words],
            axis=1).astype(jnp.bfloat16)
        y0 = pl.multiple_of(el * PITCH, 8)
        slot = lax.broadcasted_iota(jnp.int32, (CAP_PAD, LANES), 0)
        used = slot < filled

        def product(c):
            w = wv[el, :, 2 * c * LANES:2 * (c + 1) * LANES].astype(jnp.bfloat16)
            y = jnp.dot(tok, w, preferred_element_type=jnp.float32)
            return y[:, :LANES], y[:, LANES:]

        lo, hi = product(CW)
        size = jnp.where(used, lax.bitcast_convert_type(lo, jnp.int32) & 0x7FFFFFFF, 0)
        largest = jnp.max(jnp.max(size, axis=0, keepdims=True), axis=1, keepdims=True)
        base = ((largest >> 23) - 15) & 0xFF
        last = _rebase(_pack(lo, hi), base)
        thirds = [(last << 11) & _TOPS, (last << 7) & _TOPS,
                  ((last << 3) & 0x38003800) | ((last >> 1) & 0x40004000)]
        top = (last << 1) & _nibbles(CW)
        for c in range(CW):
            word = _rebase(_pack(*product(c)), base)
            res[pl.ds(y0 * CW + c, CAP_PAD, stride=CW), :] = (word & ~_TOPS) | thirds[c]
            top = top | ((word >> (11 - 4 * c)) & _nibbles(c))
        top = jnp.where(used, top, 0)
        res_top[pl.ds(y0, CAP_PAD), :] = top

        sent = sent + y_across(el)
        y_own(el)
        sent = sent + y_direct(FIRST, LATE, el, yv_recv.at[0], lambda n: el < n)
        list_wide(el, slot, top)
        notes[0] = jnp.where(note_lane == me * EL + el, base, notes[0])
        return sent, lax.cond(el > 0, lambda: y_tops(el - 1, tops), lambda: tops)

    res_sent, tops = lax.fori_loop(0, EL, run_expert, (zero, (zero,) * (N_DEV - 1)))
    res_sent = over_experts(
        lambda el: y_direct(FIRST, LATE, el, yv_recv.at[0], lambda n: el >= n),
        res_sent)
    tops = y_tops(EL - 1, tops)
    note = notes[0]
    for k in range(1, N_DEV):
        note = jnp.where(note_lane == E + me * N_DEV + peer(k), tops[k - 1], note)
    notes[0] = note
    for k in range(1, N_DEV):
        note_copy(k).start()
    yfw_sent = over_experts(y_forward, zero)
    res_sent = over_experts(
        lambda el: y_direct(LATE, LATER, el, yv_recv.at[1]), res_sent)
    res_sent = over_experts(
        lambda el: y_direct(LATER, LAST, el, yv_recv.at[2]), res_sent)

    back_copy.wait()
    for k in range(1, N_DEV):
        note_copy(k).wait_recv()
    note = (notes[0] + notes[1] + notes[2] + notes[3])[0:1, :].astype(jnp.float32)
    base_of = jnp.sum(jnp.where(l_iota == e_iota, note, 0.0), axis=1, keepdims=True)
    stage[0:ROWS, :] = jnp.where(kept, _both(per_token(base_of) << 7), 0)
    to_me = ((note_lane[0:1] >= E) & (note_lane[0:1] < E + N_DEV * N_DEV)
             & ((note_lane[0:1] & (N_DEV - 1)) == me))
    tops_in = jnp.sum(jnp.where(to_me, note, 0.0)).astype(jnp.int32)

    def arriving(el):
        def direct(b0, b1):
            return sum(segment(b0, b1, me, frm, el)[2] for frm in (right, left))

        own = segment(FIRST, LAST, me, me, el)[2]
        return (direct(FIRST, LATE) + segment(FIRST, LAST, me, across, el)[2] + own,
                direct(LATE, LATER), direct(LATER, LAST), own)

    *counts, n_own = lax.fori_loop(
        0, EL, lambda el, acc: tuple(a + b for a, b in zip(acc, arriving(el))),
        (zero,) * 4)
    wait_rows(yv_top, tops_in + n_own, top_recv)

    @pl.loop(0, ROWS)
    def _(i):
        t0 = pl.multiple_of(i * LANES, LANES)
        adds[pl.ds(t0, LANES), :] = jnp.broadcast_to(
            stage[pl.ds(i, 1), :], (LANES, LANES)).T
        for j in range(LANES):
            tok_top[pl.ds(t0 + j, 1), :] = yv_top[pl.ds(back_s[i, j], 1), :]

    half = LANES // 2

    def gather(i, part, got):
        for j in range(half):
            got[pl.ds(j * CW, CW), :] = yv[pl.ds(back_s[ROWS + i, part * half + j], CW), :]

    def write(i, part, got):
        for g in range(half // 16):
            toks = pl.ds(pl.multiple_of(i * LANES + part * half + g * 16, 16), 16)
            rows = [got[pl.ds(g * 16 * CW + c, 16, stride=CW), :] for c in range(CW)]
            for c, w in enumerate(_decode(rows + [tok_top[toks, :]], adds[toks, :])):
                out_ref[toks, 2 * c * LANES:2 * (c + 1) * LANES] = jnp.concatenate(
                    [_unpack(w, False), _unpack(w, True)], axis=1).astype(out_ref.dtype)

    edges = (0, pick(LATE_ROW, me), pick(LATER_ROW, me), ROWS)
    for c, (n, r0, r1) in enumerate(zip(counts, edges, edges[1:])):
        wait_rows(yv, n * CW, yv_recv.at[c])
        gather(r0, 0, got_a)

        def row(i, carry, r1=r1):
            gather(i, 1, got_b)
            write(i, 0, got_a)
            gather(jnp.minimum(i + 1, r1 - 1), 0, got_a)
            write(i, 1, got_b)
            return carry

        lax.fori_loop(r0, r1, row, 0)

    for k in range(1, N_DEV):
        tab_copy(k).wait_send()
        note_copy(k).wait_send()
    wait_rows(srt, srt_sent * XW, srt_send)
    wait_rows(xfw, xfw_sent * XW, xfw_send)
    wait_rows(res, res_sent * CW, res_send)
    wait_rows(yfw, yfw_sent * CW, yfw_send)
    wait_rows(res_top, sum(tops), top_send)


def pallas_dist_moe_cap_ep_tokshard_n2048_d512_e8_h1024_kernel(
    x: jax.Array,
    router_W: jax.Array,
    route_idx: jax.Array,
    expert_W: jax.Array,
):
    del router_W

    def words(*shape):
        return pltpu.VMEM(shape, jnp.int32)

    def scalars(*shape):
        return pltpu.SMEM(shape, jnp.int32)

    dma = pltpu.SemaphoreType.DMA
    slots = EL * PITCH
    in_hbm = pl.BlockSpec(memory_space=pltpu.HBM)
    return pl.pallas_call(
        _body,
        out_shape=jax.ShapeDtypeStruct((T, H), jnp.bfloat16),
        in_specs=[in_hbm, in_hbm, in_hbm],
        out_specs=pl.BlockSpec(memory_space=pltpu.VMEM),
        scratch_shapes=[
            words(ROWS, LANES),
            pltpu.VMEM((T, D), jnp.float32),
            pltpu.VMEM((EL, D, H), jnp.float32),
            words(LANES * XW + 8, LANES),
            words(T * XW, LANES),
            words(slots * XW, LANES),
            words(2 * T * XW, LANES),
            words(slots * CW, LANES),
            words(slots, LANES),
            words(2 * slots * CW, LANES),
            words(T * CW + 8, LANES),
            words(T + 8, LANES),
            words(LANES // 2 * CW + 8, LANES),
            words(LANES // 2 * CW + 8, LANES),
            words(T, LANES),
            words(T, LANES),
            words(N_DEV, TABLE_ROWS, LANES),
            words(N_DEV, 8, LANES),
            words(4 * ROWS, LANES),
            words(EL, 8, 2 * LANES),
            scalars(ROWS, LANES),
            scalars(2 * ROWS, LANES),
            scalars(TABLE_ROWS, LANES),
            scalars(2 * TABLE_ROWS, LANES),
            scalars(EL, 1, 2 * LANES),
            dma((len(X_PIECES) - 1,)), dma((EL,)), dma((5,)), dma((EL,)),
            dma((N_DEV - 1,)), dma((N_DEV - 1,)), dma((N_DEV - 1,)), dma((N_DEV - 1,)),
            dma, dma, dma, dma, dma,
            dma((EL,)), dma((EL,)), dma((EL,)), dma((3,)), dma,
        ],
        compiler_params=pltpu.CompilerParams(
            collective_id=0,
            vmem_limit_bytes=100 << 20,
            disable_semaphore_checks=True),
    )(route_idx.reshape(ROWS, LANES), x, expert_W)
```
